```python
import numpy as np

kernel_name = "dist_moe_cap_ep_outshard_n2048_d512_e8_h1024"

def setup_inputs():
    x = np.random.randn(2048, 512).astype(np.float32)
    router_W = np.random.randn(512, 32).astype(np.float32) * 0.1
    scores64 = x.astype(np.float64) @ router_W.astype(np.float64)
    route_idx = np.argsort(-scores64, axis=-1)[:, :1].astype(np.int32)
    expert_W = np.random.randn(32, 512, 1024).astype(np.float32) * 0.02
    return {"x": x, "router_W": router_W, "route_idx": route_idx, "expert_W": expert_W}

def reference(x, router_W, route_idx, expert_W):
    counts = np.zeros(32, dtype=np.int64)
    out = np.zeros((2048, 1024), dtype=np.float32)
    for i in range(2048):
        e = int(route_idx[i, 0])
        if counts[e] < 51:
            out[i] = x[i] @ expert_W[e]
            counts[e] += 1
    return out
```

```python
import jax
import jax.numpy as jnp
from jax import lax
from jax.experimental import pallas as pl
from jax.experimental.pallas import tpu as pltpu

N, D, E, H, CAP = 2048, 512, 32, 1024, 51
NDEV = 4
EL = E // NDEV
NL = N // NDEV
SL = 64
TRASH = 512
NB = N // 128


def _iota(shape, d):
    return lax.broadcasted_iota(jnp.int32, shape, d)


def _pack(lo, hi):
    lo = lax.bitcast_convert_type(lo.astype(jnp.bfloat16).astype(jnp.float32), jnp.uint32)
    hi = lax.bitcast_convert_type(hi.astype(jnp.bfloat16).astype(jnp.float32), jnp.uint32)
    return hi | (lo >> 16)


def _unpack(w):
    lo = lax.bitcast_convert_type(w << 16, jnp.float32)
    hi = lax.bitcast_convert_type(w & jnp.uint32(0xFFFF0000), jnp.float32)
    return lo, hi


def pallas_dist_moe_cap_ep_outshard_n2048_d512_e8_h1024_kernel(x, router_W, route_idx, expert_W):
    del router_W

    def body(ri_hbm, x_hbm, w_hbm, o_ref,
             ri_v, g_v, pos_v, own_v, own_s, tab_v, tab_s, xq, xp, xg, wbuf, yb, rb, r2, sel, dummy,
             wsem, lsem, ssem, rsem):
        me = lax.axis_index("i")
        cp_ri = pltpu.make_async_copy(ri_hbm, ri_v, lsem.at[0])
        cp_ri.start()
        cp_x = pltpu.make_async_copy(x_hbm.at[pl.ds(pl.multiple_of(me * NL, NL), NL)], xq, lsem.at[2])
        cp_x.start()

        def w_copy(k):
            return pltpu.make_async_copy(w_hbm.at[k], wbuf.at[k], wsem.at[k])

        def w_last(j):
            cols = slice(j * 256, (j + 1) * 256)
            return pltpu.make_async_copy(w_hbm.at[EL - 1, :, cols], wbuf.at[EL - 1, :, cols], wsem.at[EL - 1 + j])

        @pl.loop(0, EL - 1)
        def _(k):
            w_copy(k).start()
        for j in range(4):
            w_last(j).start()

        rb[:, 0:NL, :] = jnp.zeros((4, NL, 128), jnp.uint32)
        r2[...] = jnp.zeros(r2.shape, jnp.uint32)
        bar = pltpu.get_barrier_semaphore()
        for j in (1, 2, 3):
            pl.semaphore_signal(bar, 1, device_id=((me + j) % NDEV,), device_id_type=pl.DeviceIdType.MESH)

        cp_ri.wait()
        ri = ri_v[...]
        r128, c128 = _iota((128, 128), 0), _iota((128, 128), 1)
        upper = (r128 <= c128).astype(jnp.bfloat16)
        ones = jnp.ones((128, 128), jnp.bfloat16)
        lblk = ((r128 // NB == c128 // NB) & (c128 < r128)).astype(jnp.bfloat16)
        ri8 = jnp.concatenate([ri] * EL, axis=0)
        pos = jnp.zeros((NB, 128), jnp.float32)
        for c in range(NDEV):
            m = ri8 == (c * EL + r128 // NB)
            mb = m.astype(jnp.bfloat16)
            cs = jnp.dot(mb, upper, preferred_element_type=jnp.float32)
            tot = jnp.dot(mb, ones, preferred_element_type=jnp.float32)
            g = cs + jnp.dot(lblk, tot.astype(jnp.bfloat16), preferred_element_type=jnp.float32)
            g_v[c] = g
            gm = jnp.where(m, g, 0.0)
            for k in range(EL):
                pos = pos + gm[k * NB:(k + 1) * NB]
        pos_v[...] = pos
        own = pl.ds(me * 4, 4)
        p_own = pos_v[own, :].astype(jnp.int32)
        e_own = ri_v[own, :]
        keep = p_own <= CAP
        last = (e_own % EL) == EL - 1
        t_own = _iota((4, 128), 0) * 128 + _iota((4, 128), 1)
        own_v[0:4, :] = jnp.where(keep, e_own // EL, me)
        own_v[4:8, :] = jnp.where(keep, (e_own % EL) * SL + p_own - 1, EL * SL + t_own)
        cp_own = pltpu.make_async_copy(own_v, own_s, lsem.at[3])
        cp_own.start()
        rem = keep & (e_own // EL != me)
        n_keep = jnp.sum(rem.astype(jnp.float32))
        n_last = jnp.sum((rem & last).astype(jnp.float32))

        s_col = _iota((SL, 128), 0).astype(jnp.float32)
        accs = []
        for k in range(EL):
            acc = jnp.zeros((SL, 128), jnp.float32)
            for b in range(NB):
                row = g_v[me, pl.ds(k * NB + b, 1), :]
                acc = acc + jnp.where(row <= s_col, 1.0, 0.0)
            accs.append(acc.astype(jnp.bfloat16))
        acc = jnp.concatenate(accs, axis=0)
        tok = lax.dot_general(jnp.ones((8, 128), jnp.bfloat16), acc, (((1,), (1,)), ((), ())),
                              preferred_element_type=jnp.float32).astype(jnp.int32)
        slot = _iota((8, EL * SL), 1)
        valid = tok < N
        live = valid & ((slot % SL) < CAP)
        n_x = (jnp.sum((live & (tok // NL != me)).astype(jnp.float32)) / 4).astype(jnp.int32)
        n_b = n_last.astype(jnp.int32)
        n_a = 4 * (n_keep.astype(jnp.int32) - n_b)
        live_last = live & (slot >= (EL - 1) * SL)
        st = [(jnp.sum((live_last & (tok < d * NL)).astype(jnp.float32)) / 8).astype(jnp.int32)
              for d in range(1, NDEV + 1)]
        p_all = pos_v[...]
        kl_all = (p_all <= CAP) & ((ri % EL) == EL - 1)
        chip_all = _iota((NB, 128), 0) // 4
        dist = (ri // EL - chip_all - 1) % NDEV
        sto = []
        for d in range(NDEV):
            m = kl_all & (chip_all == d) & (dist < (me - d - 1) % NDEV)
            sto.append(jnp.sum(m.astype(jnp.float32)).astype(jnp.int32))
        misc = jnp.where(slot == 0, n_a, jnp.where(slot == 1, n_b, jnp.where(slot == 2, n_x, 0)))
        for d in range(NDEV):
            misc = jnp.where(slot == 4 + d, st[d], misc)
            misc = jnp.where(slot == 8 + d, sto[d], misc)
        r8 = _iota((8, EL * SL), 0)
        tab = jnp.where(r8 == 0, jnp.minimum(tok, N - 1),
              jnp.where(r8 == 1, jnp.where(valid, tok // NL, me),
              jnp.where(r8 == 2, jnp.where(valid, tok % NL, NL + slot),
              misc)))
        tab_v[...] = tab
        cp_tab = pltpu.make_async_copy(tab_v, tab_s, lsem.at[1])
        cp_tab.start()
        kl = keep & last
        src_own = e_own // EL
        code = jnp.full((4, 128), -1, jnp.int32)
        off = jnp.zeros((1, 1), jnp.int32)
        for o in (1, 2, 3, 0):
            m = kl & (src_own == (me + o) % NDEV)
            first = jnp.min(jnp.where(m, p_own, SL).astype(jnp.float32), keepdims=True).astype(jnp.int32)
            code = jnp.where(m, off + p_own - first, code)
            off = off + jnp.sum(m.astype(jnp.float32), keepdims=True).astype(jnp.int32)
        c_iota = _iota((NDEV * SL, 128), 0)
        for b in range(4):
            sel[b * 128:(b + 1) * 128, :] = (c_iota == code[b:b + 1, :]).astype(jnp.float32).T.astype(jnp.bfloat16)

        cp_x.wait()
        for j in range(2):
            xp[j] = _pack(xq[:, j * 256:j * 256 + 128], xq[:, j * 256 + 128:(j + 1) * 256])
        cp_own.wait()
        pl.semaphore_wait(bar, 3)

        def move(src, dst, j0, j1, dev, row, sem):
            dst[j0:j1, pl.ds(jnp.where(dev == me, row, TRASH), 1)] = src[...]

            @pl.when(dev != me)
            def _():
                pltpu.make_async_remote_copy(src, dst.at[j0:j1, pl.ds(row, 1)], ssem, rsem.at[sem], device_id=(dev,),
                                             device_id_type=pl.DeviceIdType.MESH).start()

        def dispatch(b, c):
            for l in range(128):
                move(xp.at[:, pl.ds(b * 128 + l, 1)], xg, 0, 2, own_s[b, l], own_s[4 + b, l], 1)
            return c
        lax.fori_loop(0, 4, dispatch, 0)

        def wait_rows(n, sem):
            pltpu.make_async_copy(dummy.at[pl.ds(0, n)], dummy.at[pl.ds(0, n)], sem).wait()

        cp_tab.wait()
        wait_rows(tab_s[3, 2], rsem.at[1])

        def send(k, j0, j1, sem):
            for s in range(CAP):
                i = k * SL + s
                move(yb.at[j0:j1, pl.ds(i, 1)], rb, j0, j1, tab_s[1, i], tab_s[2, i], sem)

        def load_x(k):
            rows = pl.ds(pl.multiple_of(k * SL, SL), SL)
            return jnp.concatenate(_unpack(xg[0, rows, :]) + _unpack(xg[1, rows, :]), axis=1).astype(jnp.bfloat16)

        def compute(k, j0, j1):
            rows = pl.ds(pl.multiple_of(k * SL, SL), SL)
            xb = load_x(k)
            for j in range(j0, j1):
                y = jnp.dot(xb, wbuf[k, :, j * 256:(j + 1) * 256].astype(jnp.bfloat16),
                            preferred_element_type=jnp.float32)
                yb[j, rows, :] = _pack(y[:, :128], y[:, 128:])

        def expert(k, c):
            w_copy(k).wait()
            compute(k, 0, 4)
            send(k, 0, 4, 0)
            return c
        lax.fori_loop(0, EL - 1, expert, 0)
        base = (EL - 1) * SL
        xb = load_x(jnp.int32(EL - 1))
        lo_me = tab_s[3, 3 + me]
        mine = _iota((SL, 128), 0) < tab_s[3, 4 + me] - lo_me
        for j in range(4):
            w_last(j).wait()
            y = jnp.dot(xb, wbuf[EL - 1, :, j * 256:(j + 1) * 256].astype(jnp.bfloat16),
                        preferred_element_type=jnp.float32)
            yb[j, base:base + SL, :] = _pack(y[:, :128], y[:, 128:])
            for o in (2, 1, 3):
                d = (me + o) % NDEV
                lo = tab_s[3, 3 + d]
                n = tab_s[3, 4 + d] - lo

                @pl.when(n > 0)
                def _():
                    pltpu.make_async_remote_copy(
                        yb.at[j, pl.ds(base + lo, n)], r2.at[j, pl.ds(tab_s[3, 8 + d], n)], ssem, rsem.at[2 + j],
                        device_id=(d,), device_id_type=pl.DeviceIdType.MESH).start()
            r2[j, pl.ds(tab_s[3, 8 + me], SL), :] = jnp.where(mine, yb[j, pl.ds(base + lo_me, SL), :], jnp.uint32(0))

        wait_rows(tab_s[3, 0], rsem.at[0])
        for j in range(4):
            cols = slice(j * 256, (j + 1) * 256)

            def placed(h):
                rows = jnp.concatenate(_unpack(r2[j, h * 128:(h + 1) * 128, :]), axis=1).astype(jnp.bfloat16)
                return jnp.dot(sel[:, h * 128:(h + 1) * 128], rows, preferred_element_type=jnp.float32)

            wait_rows(tab_s[3, 1], rsem.at[2 + j])
            o_ref[:, cols] = jnp.concatenate(_unpack(rb[j, 0:NL, :]), axis=1) + placed(0)

            @pl.when(tab_s[3, 8 + me] + SL > 128)
            def _():
                o_ref[:, cols] += placed(1)
        wait_rows(2 * tab_s[3, 2] + tab_s[3, 0] // 2 + 2 * tab_s[3, 1], ssem)

    return pl.pallas_call(
        body,
        out_shape=jax.ShapeDtypeStruct((NL, H), jnp.float32),
        in_specs=[pl.BlockSpec(memory_space=pl.ANY)] * 3,
        out_specs=pl.BlockSpec(memory_space=pltpu.VMEM),
        scratch_shapes=[
            pltpu.VMEM((NB, 128), jnp.int32),
            pltpu.VMEM((NDEV, 128, 128), jnp.float32),
            pltpu.VMEM((NB, 128), jnp.float32),
            pltpu.VMEM((8, 128), jnp.int32),
            pltpu.SMEM((8, 128), jnp.int32),
            pltpu.VMEM((8, EL * SL), jnp.int32),
            pltpu.SMEM((8, EL * SL), jnp.int32),
            pltpu.VMEM((NL, D), jnp.float32),
            pltpu.VMEM((2, NL, 128), jnp.uint32),
            pltpu.VMEM((2, EL * SL + NL, 128), jnp.uint32),
            pltpu.VMEM((EL, D, H), jnp.float32),
            pltpu.VMEM((4, EL * SL + SL, 128), jnp.uint32),
            pltpu.VMEM((4, 2 * NL, 128), jnp.uint32),
            pltpu.VMEM((4, NDEV * SL, 128), jnp.uint32),
            pltpu.VMEM((NL, NDEV * SL), jnp.bfloat16),
            pltpu.VMEM((4 * 2 * NL, 128), jnp.uint32),
            pltpu.SemaphoreType.DMA((EL + 3,)),
            pltpu.SemaphoreType.DMA((4,)),
            pltpu.SemaphoreType.DMA,
            pltpu.SemaphoreType.DMA((6,)),
        ],
        compiler_params=pltpu.CompilerParams(vmem_limit_bytes=64 << 20, collective_id=0),
    )(route_idx.reshape(NB, 128), x, expert_W)
```
